```python
import numpy as np

kernel_name = "dist_ar_xy_y_m1024_n512"

def setup_inputs():
    return {"x": np.random.randn(2048, 512).astype(np.float32)}

def reference(x: np.ndarray) -> np.ndarray:
    return x.reshape(2, 1024, 512).sum(axis=0)
```

```python
import jax
import jax.numpy as jnp
from jax import lax
from jax.experimental import pallas as pl
from jax.experimental.pallas import tpu as pltpu

_MESH = pl.DeviceIdType.MESH

_BR = 16
_UC = 128
_E_UNITS = 2
_D_UNITS = 10
_PRE = (1, 2, 5)
_X_TAIL = (2, 1)


def pallas_dist_ar_xy_y_m1024_n512_kernel(x: jax.Array):
    m, n = x.shape
    half = m // 2
    nb = half // _BR
    upb = n // _UC
    e = _E_UNITS
    u = nb * upb - _D_UNITS
    fb, fc = divmod(u, upb)
    assert 0 < e < upb and 0 < fc and fb + 2 <= nb

    f_units = [(k // upb * _BR, _BR, k % upb * _UC, _UC) for k in range(e, u)]
    e_tiles = [(r, 8, c * _UC, _UC) for c in range(e) for r in (0, 8)]
    bulk = fb - 1 - sum(_X_TAIL)
    f_rects = [(0, _BR, e * _UC, n - e * _UC), (_BR, bulk * _BR, 0, n)]
    for t in _X_TAIL:
        f_rects.append((f_rects[-1][0] + f_rects[-1][1], t * _BR, 0, n))
    f_rects.append((fb * _BR, _BR, 0, fc * _UC))
    d_head = (fb * _BR, _BR, fc * _UC, n - fc * _UC)
    d_pieces = [(1, d_head), (1, ((fb + 1) * _BR, half - (fb + 1) * _BR, 0, n)), (0, d_head)]
    d_pieces += [(0, (b * _BR, _BR, 0, n)) for b in range(fb + 1, nb)]
    groups = list(_PRE) + [nb - sum(_PRE)]
    group_off = [sum(groups[:i]) for i in range(len(groups))]

    def f_group(k):
        row = f_units[k][0]
        return [i for i, r in enumerate(f_rects) if r[0] <= row < r[0] + r[1]][0]

    def body(x_hbm, out, xs, sbuf, rbuf, ebuf, ld_sem, yf_send, yf_recv, yd_send, yd_recv,
             xf_send, xf_recv, e_send, ey_recv, ex_recv, last_in):
        mx, my = lax.axis_index("x"), lax.axis_index("y")
        ynbr, xnbr = (mx, 1 - my), (1 - mx, my)
        base = [pl.multiple_of(mx * half, half), pl.multiple_of((1 - mx) * half, half)]

        def idx(h, rect):
            return (pl.ds(base[h] + rect[0], rect[1]), pl.ds(rect[2], rect[3]))

        def load(h, row0, rows, s):
            sl = pl.ds(base[h] + row0, rows)
            return pltpu.make_async_copy(x_hbm.at[sl], xs.at[sl], ld_sem.at[s])

        def rdma(src, dst, send_sem, recv_sem, dev):
            return pltpu.make_async_remote_copy(
                src, dst, send_sem, recv_sem, device_id=dev, device_id_type=_MESH)

        def ey(i):
            r, rows, c, cols = e_tiles[i]
            return rdma(x_hbm.at[idx(0, e_tiles[i])], ebuf.at[0, pl.ds(r, rows), pl.ds(c, cols)],
                        e_send.at[0], ey_recv.at[i], ynbr)

        def ex(i):
            r, rows, c, cols = e_tiles[i]
            return rdma(ebuf.at[0, pl.ds(r, rows), pl.ds(c, cols)],
                        ebuf.at[1, pl.ds(r, rows), pl.ds(c, cols)], e_send.at[1], ex_recv, xnbr)

        def yf(k):
            sl = idx(0, f_units[k])
            return rdma(sbuf.at[sl], rbuf.at[sl], yf_send.at[f_group(k)], yf_recv.at[k], ynbr)

        def xf(k):
            sl = idx(0, f_units[k])
            g = f_group(k)
            return rdma(rbuf.at[sl], rbuf.at[sl], xf_send.at[g], xf_recv.at[g], xnbr)

        def yd(i):
            sl = idx(*d_pieces[i])
            return rdma(sbuf.at[sl], rbuf.at[sl], yd_send.at[i], yd_recv.at[i], ynbr)

        def convert(h, row0, rows):
            sl = idx(h, (row0, rows, 0, n))
            sbuf[sl] = xs[sl].astype(jnp.bfloat16)

        def add(h, rect):
            sl = idx(h, rect)
            out[sl] = xs[sl] + rbuf[sl].astype(jnp.float32)

        def send_block(b):
            convert(0, b * _BR, _BR)
            for k, r in enumerate(f_units):
                if r[0] == b * _BR:
                    yf(k).start()

        loads = [load(0, group_off[i] * _BR, groups[i] * _BR, i) for i in range(len(groups))]
        load_other_d = load(1, fb * _BR, half - fb * _BR, len(groups))
        load_other_f = load(1, 0, fb * _BR, len(groups) + 1)

        barrier = pltpu.get_barrier_semaphore()
        is_last = jnp.logical_and(mx == 1, my == 1)

        @pl.when(jnp.logical_not(is_last))
        def _():
            pl.semaphore_signal(barrier, 1, device_id=ynbr, device_id_type=_MESH)
            pl.semaphore_signal(barrier, 1, device_id=xnbr, device_id_type=_MESH)

        for c in loads + [load_other_d, load_other_f]:
            c.start()

        @pl.when(mx == my)
        def _():
            pl.semaphore_wait(barrier, 2)

        @pl.when(mx != my)
        def _():
            pl.semaphore_wait(barrier, 1)

        @pl.when(jnp.logical_and(mx == 1, my == 0))
        def _():
            pl.semaphore_wait(last_in, 1)

        for i in range(len(e_tiles)):
            ey(i).start()

        @pl.when(is_last)
        def _():
            pl.semaphore_signal(last_in, 1, device_id=ynbr, device_id_type=_MESH)
            pl.semaphore_signal(last_in, 1, device_id=xnbr, device_id_type=_MESH)

        for i in range(len(_PRE)):
            loads[i].wait()
            for b in range(group_off[i], group_off[i] + groups[i]):
                send_block(b)

        @pl.when(jnp.logical_and(mx == 0, my == 1))
        def _():
            pl.semaphore_wait(last_in, 1)

        def send_first():
            loads[-1].wait()
            send_block(sum(_PRE))

        def send_other_d():
            load_other_d.wait()
            convert(1, fb * _BR, half - fb * _BR)
            yd(0).start()
            yd(1).start()

        def send_my_d():
            convert(0, (fb + 1) * _BR, half - (fb + 1) * _BR)
            for i in range(2, len(d_pieces)):
                yd(i).start()

        todo = [send_first]
        todo += [lambda b=b: send_block(b) for b in range(sum(_PRE) + 1, fb + 1)]
        todo += [send_other_d, send_my_d]

        for i in range(len(e_tiles)):
            ey(i).wait_recv()
            ex(i).start()
        for k, r in enumerate(f_units):
            yf(k).wait_recv()
            xf(k).start()
            if todo and (k == 0 or r[2] == 0):
                todo.pop(0)()
        assert not todo

        e_rect = (0, _BR, 0, e * _UC)
        out[idx(0, e_rect)] = xs[idx(0, e_rect)] + ebuf[0]
        for r in f_rects:
            add(0, r)
        load_other_f.wait()
        rdma(ebuf.at[1], ebuf.at[1], e_send.at[1], ex_recv, xnbr).wait_recv()
        out[idx(1, e_rect)] = xs[idx(1, e_rect)] + ebuf[1]

        def finish_x(g):
            sl = idx(1, f_rects[g])
            rdma(rbuf.at[sl], rbuf.at[sl], xf_send.at[g], xf_recv.at[g], xnbr).wait_recv()
            add(1, f_rects[g])

        def finish_d(i):
            yd(i).wait_recv()
            add(*d_pieces[i])

        def finish_sends():
            rdma(x_hbm.at[idx(0, e_rect)], ebuf.at[0], e_send.at[0], ex_recv, ynbr).wait_send()
            rdma(ebuf.at[0], ebuf.at[1], e_send.at[1], ex_recv, xnbr).wait_send()
            for g, r in enumerate(f_rects):
                sl = idx(0, r)
                rdma(sbuf.at[sl], rbuf.at[sl], yf_send.at[g], xf_recv.at[g], ynbr).wait_send()
                rdma(rbuf.at[sl], rbuf.at[sl], xf_send.at[g], xf_recv.at[g], xnbr).wait_send()
            for i in range(len(d_pieces)):
                yd(i).wait_send()

        nx, nd = len(f_rects), len(d_pieces)
        finish_x(0)
        finish_x(1)
        for i in range(nd - 2):
            finish_d(i)
        for g in range(2, nx - 1):
            finish_x(g)
        finish_d(nd - 2)
        finish_sends()
        finish_d(nd - 1)
        finish_x(nx - 1)

    dma = pltpu.SemaphoreType.DMA
    return pl.pallas_call(
        body,
        out_shape=jax.ShapeDtypeStruct((m, n), x.dtype),
        in_specs=[pl.BlockSpec(memory_space=pl.ANY)],
        out_specs=pl.BlockSpec(memory_space=pltpu.VMEM),
        scratch_shapes=[
            pltpu.VMEM((m, n), jnp.float32),
            pltpu.VMEM((m, n), jnp.bfloat16),
            pltpu.VMEM((m, n), jnp.bfloat16),
            pltpu.VMEM((2, _BR, e * _UC), jnp.float32),
            dma((len(groups) + 2,)),
            dma((len(f_rects),)),
            dma((len(f_units),)),
            dma((len(d_pieces),)),
            dma((len(d_pieces),)),
            dma((len(f_rects),)),
            dma((len(f_rects),)),
            dma((2,)),
            dma((len(e_tiles),)),
            dma,
            pltpu.SemaphoreType.REGULAR,
        ],
        compiler_params=pltpu.CompilerParams(collective_id=0, disable_semaphore_checks=True),
    )(x)
```

```python
import jax
import jax.numpy as jnp
from jax import lax
from jax.experimental import pallas as pl
from jax.experimental.pallas import tpu as pltpu

_MESH = pl.DeviceIdType.MESH

_BR = 16
_UC = 128
_E_UNITS = 1
_D_UNITS = 10
_PRE = (2, 5)
_X_TAIL = (2, 1)


def pallas_dist_ar_xy_y_m1024_n512_kernel(x: jax.Array):
    m, n = x.shape
    half = m // 2
    nb = half // _BR
    upb = n // _UC
    e = _E_UNITS
    u = nb * upb - _D_UNITS
    fb, fc = divmod(u, upb)
    assert 0 < e < upb and 0 < fc and fb + 2 <= nb

    f_units = [(k // upb * _BR, _BR, k % upb * _UC, _UC) for k in range(e, u)]
    e_tiles = [(r, 8, c * _UC, _UC) for c in range(e) for r in (0, 8)]
    bulk = fb - 1 - sum(_X_TAIL)
    f_rects = [(0, _BR, e * _UC, n - e * _UC), (_BR, bulk * _BR, 0, n)]
    for t in _X_TAIL:
        f_rects.append((f_rects[-1][0] + f_rects[-1][1], t * _BR, 0, n))
    f_rects.append((fb * _BR, _BR, 0, fc * _UC))
    d_head = (fb * _BR, _BR, fc * _UC, n - fc * _UC)
    d_pieces = [(1, d_head), (1, ((fb + 1) * _BR, half - (fb + 1) * _BR, 0, n)), (0, d_head)]
    d_pieces += [(0, (b * _BR, _BR, 0, n)) for b in range(fb + 1, nb)]
    e_rect = (0, _BR, 0, e * _UC)
    n_pre = 1 + sum(_PRE)
    ld_rects = [(0, r) for r in f_units[:upb - e]]
    for i, t in enumerate(list(_PRE) + [nb - n_pre]):
        ld_rects.append((0, ((1 + sum(_PRE[:i])) * _BR, t * _BR, 0, n)))
    ld_rects += [(1, (fb * _BR, half - fb * _BR, 0, n)), (0, e_rect), (1, (0, fb * _BR, 0, n))]

    def f_group(k):
        row = f_units[k][0]
        return [i for i, r in enumerate(f_rects) if r[0] <= row < r[0] + r[1]][0]

    def body(x_hbm, out, xs, sbuf, rbuf, ebuf, ld_sem, yf_send, yf_recv, yd_send, yd_recv,
             xf_send, xf_recv, e_send, ey_recv, ex_recv, last_in):
        mx, my = lax.axis_index("x"), lax.axis_index("y")
        ynbr, xnbr = (mx, 1 - my), (1 - mx, my)
        base = [pl.multiple_of(mx * half, half), pl.multiple_of((1 - mx) * half, half)]

        def idx(h, rect):
            return (pl.ds(base[h] + rect[0], rect[1]), pl.ds(rect[2], rect[3]))

        def load(i):
            sl = idx(*ld_rects[i])
            return pltpu.make_async_copy(x_hbm.at[sl], xs.at[sl], ld_sem.at[i])

        def rdma(src, dst, send_sem, recv_sem, dev):
            return pltpu.make_async_remote_copy(
                src, dst, send_sem, recv_sem, device_id=dev, device_id_type=_MESH)

        def ey(i):
            r, rows, c, cols = e_tiles[i]
            return rdma(x_hbm.at[idx(0, e_tiles[i])], ebuf.at[0, pl.ds(r, rows), pl.ds(c, cols)],
                        e_send.at[0], ey_recv.at[i], ynbr)

        def ex(i):
            r, rows, c, cols = e_tiles[i]
            return rdma(ebuf.at[0, pl.ds(r, rows), pl.ds(c, cols)],
                        ebuf.at[1, pl.ds(r, rows), pl.ds(c, cols)], e_send.at[1], ex_recv, xnbr)

        def yf(k):
            sl = idx(0, f_units[k])
            return rdma(sbuf.at[sl], rbuf.at[sl], yf_send.at[f_group(k)], yf_recv.at[k], ynbr)

        def xf(k):
            sl = idx(0, f_units[k])
            g = f_group(k)
            return rdma(rbuf.at[sl], rbuf.at[sl], xf_send.at[g], xf_recv.at[g], xnbr)

        def yd(i):
            sl = idx(*d_pieces[i])
            return rdma(sbuf.at[sl], rbuf.at[sl], yd_send.at[i], yd_recv.at[i], ynbr)

        def convert(h, rect):
            sl = idx(h, rect)
            sbuf[sl] = xs[sl].astype(jnp.bfloat16)

        def add(h, rect):
            sl = idx(h, rect)
            out[sl] = xs[sl] + rbuf[sl].astype(jnp.float32)

        def send_block(b):
            convert(0, (b * _BR, _BR, 0, n))
            for k, r in enumerate(f_units):
                if r[0] == b * _BR:
                    yf(k).start()

        barrier = pltpu.get_barrier_semaphore()
        is_last = jnp.logical_and(mx == 1, my == 1)

        @pl.when(jnp.logical_not(is_last))
        def _():
            pl.semaphore_signal(barrier, 1, device_id=ynbr, device_id_type=_MESH)
            pl.semaphore_signal(barrier, 1, device_id=xnbr, device_id_type=_MESH)

        for i in range(len(ld_rects)):
            load(i).start()

        @pl.when(mx == my)
        def _():
            pl.semaphore_wait(barrier, 2)

        @pl.when(mx != my)
        def _():
            pl.semaphore_wait(barrier, 1)

        @pl.when(jnp.logical_and(mx == 1, my == 0))
        def _():
            pl.semaphore_wait(last_in, 1)

        for i in range(len(e_tiles)):
            ey(i).start()

        @pl.when(is_last)
        def _():
            pl.semaphore_signal(last_in, 1, device_id=ynbr, device_id_type=_MESH)
            pl.semaphore_signal(last_in, 1, device_id=xnbr, device_id_type=_MESH)

        for k in range(upb - e):
            load(k).wait()
            convert(0, f_units[k])
            yf(k).start()
        for i in range(upb - e, upb - e + len(_PRE)):
            load(i).wait()
            row0, rows = ld_rects[i][1][:2]
            for b in range(row0 // _BR, (row0 + rows) // _BR):
                send_block(b)
        ld_rest, ld_other_d, ld_e, ld_other_f = range(len(ld_rects) - 4, len(ld_rects))

        @pl.when(jnp.logical_and(mx == 0, my == 1))
        def _():
            pl.semaphore_wait(last_in, 1)

        def send_first():
            load(ld_rest).wait()
            send_block(n_pre)

        def send_other_d():
            load(ld_other_d).wait()
            convert(*ld_rects[ld_other_d])
            yd(0).start()
            yd(1).start()

        def send_my_d():
            convert(0, d_pieces[1][1])
            for i in range(2, len(d_pieces)):
                yd(i).start()

        todo = [send_first]
        todo += [lambda b=b: send_block(b) for b in range(n_pre + 1, fb + 1)]
        todo += [send_other_d, send_my_d]

        for i in range(len(e_tiles)):
            ey(i).wait_recv()
            ex(i).start()
        for k, r in enumerate(f_units):
            yf(k).wait_recv()
            xf(k).start()
            if todo and (k == 0 or r[2] == 0):
                todo.pop(0)()
        assert not todo

        load(ld_e).wait()
        out[idx(0, e_rect)] = xs[idx(0, e_rect)] + ebuf[0]
        for r in f_rects:
            add(0, r)
        load(ld_other_f).wait()
        rdma(ebuf.at[1], ebuf.at[1], e_send.at[1], ex_recv, xnbr).wait_recv()
        out[idx(1, e_rect)] = xs[idx(1, e_rect)] + ebuf[1]

        def finish_x(g):
            sl = idx(1, f_rects[g])
            rdma(rbuf.at[sl], rbuf.at[sl], xf_send.at[g], xf_recv.at[g], xnbr).wait_recv()
            add(1, f_rects[g])

        def finish_d(i):
            yd(i).wait_recv()
            add(*d_pieces[i])

        def finish_sends():
            rdma(x_hbm.at[idx(0, e_rect)], ebuf.at[0], e_send.at[0], ex_recv, ynbr).wait_send()
            rdma(ebuf.at[0], ebuf.at[1], e_send.at[1], ex_recv, xnbr).wait_send()
            for g, r in enumerate(f_rects):
                sl = idx(0, r)
                rdma(sbuf.at[sl], rbuf.at[sl], yf_send.at[g], xf_recv.at[g], ynbr).wait_send()
                rdma(rbuf.at[sl], rbuf.at[sl], xf_send.at[g], xf_recv.at[g], xnbr).wait_send()
            for i in range(len(d_pieces)):
                yd(i).wait_send()

        nx, nd = len(f_rects), len(d_pieces)
        finish_x(0)
        finish_x(1)
        for i in range(nd - 2):
            finish_d(i)
        for g in range(2, nx - 1):
            finish_x(g)
        finish_d(nd - 2)
        finish_sends()
        finish_d(nd - 1)
        finish_x(nx - 1)

    params = dict(collective_id=0)
    if hasattr(pltpu.CompilerParams, "disable_semaphore_checks"):
        params["disable_semaphore_checks"] = True

    dma = pltpu.SemaphoreType.DMA
    return pl.pallas_call(
        body,
        out_shape=jax.ShapeDtypeStruct((m, n), x.dtype),
        in_specs=[pl.BlockSpec(memory_space=pl.ANY)],
        out_specs=pl.BlockSpec(memory_space=pltpu.VMEM),
        scratch_shapes=[
            pltpu.VMEM((m, n), jnp.float32),
            pltpu.VMEM((m, n), jnp.bfloat16),
            pltpu.VMEM((m, n), jnp.bfloat16),
            pltpu.VMEM((2, _BR, e * _UC), jnp.float32),
            dma((len(ld_rects),)),
            dma((len(f_rects),)),
            dma((len(f_units),)),
            dma((len(d_pieces),)),
            dma((len(d_pieces),)),
            dma((len(f_rects),)),
            dma((len(f_rects),)),
            dma((2,)),
            dma((len(e_tiles),)),
            dma,
            pltpu.SemaphoreType.REGULAR,
        ],
        compiler_params=pltpu.CompilerParams(**params),
    )(x)
```

```python
import functools

import jax
import jax.numpy as jnp
from jax import lax
from jax.experimental import pallas as pl
from jax.experimental.pallas import tpu as pltpu

_MESH = pl.DeviceIdType.MESH

_BR = 16
_UC = 128
_E_UNITS = 1
_D_UNITS = 10
_GROUPS = (2, 5, 8)
_LEAD = 8
_X_TAIL = (2, 1)


def pallas_dist_ar_xy_y_m1024_n512_kernel(x: jax.Array):
    m, n = x.shape
    half = m // 2
    nb = half // _BR
    upb = n // _UC
    e = _E_UNITS
    u = nb * upb - _D_UNITS
    fb, fc = divmod(u, upb)
    assert 0 < e < upb and 0 < fc and fb + 2 <= nb

    f_units = [(k // upb * _BR, _BR, k % upb * _UC, _UC) for k in range(e, u)]
    e_tiles = [(r, 8, c * _UC, _UC) for c in range(e) for r in (0, 8)]
    bulk = fb - 1 - sum(_X_TAIL)
    f_rects = [(0, _BR, e * _UC, n - e * _UC), (_BR, bulk * _BR, 0, n)]
    for t in _X_TAIL:
        f_rects.append((f_rects[-1][0] + f_rects[-1][1], t * _BR, 0, n))
    f_rects.append((fb * _BR, _BR, 0, fc * _UC))
    d_head = (fb * _BR, _BR, fc * _UC, n - fc * _UC)
    d_pieces = [(1, d_head), (1, ((fb + 1) * _BR, half - (fb + 1) * _BR, 0, n)), (0, d_head)]
    d_pieces += [(0, (b * _BR, _BR, 0, n)) for b in range(fb + 1, nb)]
    e_rect = (0, _BR, 0, e * _UC)
    ld_rects = [(0, r) for r in f_units[:upb - e]]
    ld_of_block = {}
    for i, t in enumerate(list(_GROUPS) + [nb - 1 - sum(_GROUPS)]):
        ld_of_block[1 + sum(_GROUPS[:i])] = len(ld_rects)
        ld_rects.append((0, ((1 + sum(_GROUPS[:i])) * _BR, t * _BR, 0, n)))
    assert max(ld_of_block) <= fb
    ld_rects += [(1, (fb * _BR, half - fb * _BR, 0, n)), (0, e_rect), (1, (0, fb * _BR, 0, n))]
    ld_other_d, ld_e, ld_other_f = range(len(ld_rects) - 3, len(ld_rects))

    def f_group(k):
        row = f_units[k][0]
        return [i for i, r in enumerate(f_rects) if r[0] <= row < r[0] + r[1]][0]

    def run(x_hbm, out, xs, sbuf, rbuf, ebuf, ld_sem, yf_send, yf_recv, yd_send, yd_recv,
            xf_send, xf_recv, e_send, ey_recv, ex_recv, last_in):
        mx, my = lax.axis_index("x"), lax.axis_index("y")
        ynbr, xnbr = (mx, 1 - my), (1 - mx, my)
        base = [pl.multiple_of(mx * half, half), pl.multiple_of((1 - mx) * half, half)]

        def idx(h, rect):
            return (pl.ds(base[h] + rect[0], rect[1]), pl.ds(rect[2], rect[3]))

        def load(i):
            sl = idx(*ld_rects[i])
            return pltpu.make_async_copy(x_hbm.at[sl], xs.at[sl], ld_sem.at[i])

        def rdma(src, dst, send_sem, recv_sem, dev):
            return pltpu.make_async_remote_copy(
                src, dst, send_sem, recv_sem, device_id=dev, device_id_type=_MESH)

        def ey(i):
            r, rows, c, cols = e_tiles[i]
            return rdma(x_hbm.at[idx(0, e_tiles[i])], ebuf.at[0, pl.ds(r, rows), pl.ds(c, cols)],
                        e_send.at[0], ey_recv.at[i], ynbr)

        def ex(i):
            r, rows, c, cols = e_tiles[i]
            return rdma(ebuf.at[0, pl.ds(r, rows), pl.ds(c, cols)],
                        ebuf.at[1, pl.ds(r, rows), pl.ds(c, cols)], e_send.at[1], ex_recv, xnbr)

        def yf(k):
            sl = idx(0, f_units[k])
            return rdma(sbuf.at[sl], rbuf.at[sl], yf_send.at[f_group(k)], yf_recv.at[k], ynbr)

        def xf(k):
            sl = idx(0, f_units[k])
            g = f_group(k)
            return rdma(rbuf.at[sl], rbuf.at[sl], xf_send.at[g], xf_recv.at[g], xnbr)

        def yd(i):
            sl = idx(*d_pieces[i])
            return rdma(sbuf.at[sl], rbuf.at[sl], yd_send.at[i], yd_recv.at[i], ynbr)

        def convert(h, rect):
            sl = idx(h, rect)
            sbuf[sl] = xs[sl].astype(jnp.bfloat16)

        def add(h, rect):
            sl = idx(h, rect)
            out[sl] = xs[sl] + rbuf[sl].astype(jnp.float32)

        def send_block(b):
            if b in ld_of_block:
                load(ld_of_block[b]).wait()
            convert(0, (b * _BR, _BR, 0, n))
            for k, r in enumerate(f_units):
                if r[0] == b * _BR:
                    yf(k).start()

        barrier = pltpu.get_barrier_semaphore()
        is_last = jnp.logical_and(mx == 1, my == 1)

        @pl.when(jnp.logical_not(is_last))
        def _():
            pl.semaphore_signal(barrier, 1, device_id=ynbr, device_id_type=_MESH)
            pl.semaphore_signal(barrier, 1, device_id=xnbr, device_id_type=_MESH)

        for i in range(len(ld_rects)):
            load(i).start()

        @pl.when(mx == my)
        def _():
            pl.semaphore_wait(barrier, 2)

        @pl.when(mx != my)
        def _():
            pl.semaphore_wait(barrier, 1)

        @pl.when(jnp.logical_and(mx == 1, my == 0))
        def _():
            pl.semaphore_wait(last_in, 1)

        for i in range(len(e_tiles)):
            ey(i).start()

        @pl.when(is_last)
        def _():
            pl.semaphore_signal(last_in, 1, device_id=ynbr, device_id_type=_MESH)
            pl.semaphore_signal(last_in, 1, device_id=xnbr, device_id_type=_MESH)

        for k in range(upb - e):
            load(k).wait()
            convert(0, f_units[k])
            yf(k).start()
        for b in range(1, _LEAD):
            send_block(b)

        @pl.when(jnp.logical_and(mx == 0, my == 1))
        def _():
            pl.semaphore_wait(last_in, 1)

        def send_other_d():
            load(ld_other_d).wait()
            convert(*ld_rects[ld_other_d])
            yd(0).start()
            yd(1).start()

        def send_my_d():
            convert(0, d_pieces[1][1])
            for i in range(2, len(d_pieces)):
                yd(i).start()

        todo = [lambda b=b: send_block(b) for b in range(_LEAD, fb + 1)]
        todo += [send_other_d, send_my_d]

        for i in range(len(e_tiles)):
            ey(i).wait_recv()
            ex(i).start()
        for k, r in enumerate(f_units):
            yf(k).wait_recv()
            xf(k).start()
            if todo and (k == 0 or r[2] == 0):
                todo.pop(0)()
        assert not todo

        load(ld_e).wait()
        out[idx(0, e_rect)] = xs[idx(0, e_rect)] + ebuf[0]
        for r in f_rects:
            add(0, r)
        load(ld_other_f).wait()
        rdma(ebuf.at[1], ebuf.at[1], e_send.at[1], ex_recv, xnbr).wait_recv()
        out[idx(1, e_rect)] = xs[idx(1, e_rect)] + ebuf[1]

        def finish_x(g):
            sl = idx(1, f_rects[g])
            rdma(rbuf.at[sl], rbuf.at[sl], xf_send.at[g], xf_recv.at[g], xnbr).wait_recv()
            add(1, f_rects[g])

        def finish_d(i):
            yd(i).wait_recv()
            add(*d_pieces[i])

        def finish_sends():
            rdma(x_hbm.at[idx(0, e_rect)], ebuf.at[0], e_send.at[0], ex_recv, ynbr).wait_send()
            rdma(ebuf.at[0], ebuf.at[1], e_send.at[1], ex_recv, xnbr).wait_send()
            for g, r in enumerate(f_rects):
                sl = idx(0, r)
                rdma(sbuf.at[sl], rbuf.at[sl], yf_send.at[g], xf_recv.at[g], ynbr).wait_send()
                rdma(rbuf.at[sl], rbuf.at[sl], xf_send.at[g], xf_recv.at[g], xnbr).wait_send()
            for i in range(len(d_pieces)):
                yd(i).wait_send()

        nx, nd = len(f_rects), len(d_pieces)
        finish_x(0)
        finish_x(1)
        for i in range(nd - 2):
            finish_d(i)
        for g in range(2, nx - 1):
            finish_x(g)
        finish_d(nd - 2)
        finish_sends()
        finish_d(nd - 1)
        finish_x(nx - 1)

    def body(*refs):
        dma = pltpu.SemaphoreType.DMA
        pl.run_scoped(
            functools.partial(run, *refs),
            ld_sem=dma((len(ld_rects),)),
            yf_send=dma((len(f_rects),)),
            yf_recv=dma((len(f_units),)),
            yd_send=dma((len(d_pieces),)),
            yd_recv=dma((len(d_pieces),)),
            xf_send=dma((len(f_rects),)),
            xf_recv=dma((len(f_rects),)),
            e_send=dma((2,)),
            ey_recv=dma((len(e_tiles),)),
            ex_recv=dma,
            last_in=pltpu.SemaphoreType.REGULAR,
        )

    return pl.pallas_call(
        body,
        out_shape=jax.ShapeDtypeStruct((m, n), x.dtype),
        in_specs=[pl.BlockSpec(memory_space=pl.ANY)],
        out_specs=pl.BlockSpec(memory_space=pltpu.VMEM),
        scratch_shapes=[
            pltpu.VMEM((m, n), jnp.float32),
            pltpu.VMEM((m, n), jnp.bfloat16),
            pltpu.VMEM((m, n), jnp.bfloat16),
            pltpu.VMEM((2, _BR, e * _UC), jnp.float32),
        ],
        compiler_params=pltpu.CompilerParams(collective_id=0),
    )(x)
```
